```python
import numpy as np

kernel_name = "dist_rmsnorm_colshard_i_m768_n512"

def setup_inputs():
    x = np.random.randn(768, 2048).astype(np.float32)
    gamma = np.random.randn(2048).astype(np.float32)
    return {"x": x, "gamma": gamma}

def reference(x: np.ndarray, gamma: np.ndarray) -> np.ndarray:
    eps = 1e-5
    rms = np.sqrt(np.mean(x * x, axis=1, keepdims=True) + eps)
    return gamma * x / rms
```

```python
import jax
import jax.numpy as jnp
from jax import lax
from jax.experimental import pallas as pl
from jax.experimental.pallas import tpu as pltpu

N_DEV = 4
EPS = 1e-5
LANES = 128


def pallas_dist_rmsnorm_colshard_i_m768_n512_kernel(
    x: jax.Array,
    gamma: jax.Array,
):
    m, n = x.shape
    rows = LANES
    nch = m // rows
    assert m % rows == 0 and n % LANES == 0
    n_glob = n * N_DEV
    nj = n // LANES
    g2 = gamma.reshape(1, n)

    def body(x_ref, g_ref, o_ref, xbuf, gbuf, sbuf, rbuf,
             in_sems, g_sem, send_sems, recv_sems):
        me = lax.axis_index("i")
        loads = []
        for c in range(nch):
            cp = pltpu.make_async_copy(
                x_ref.at[pl.ds(c * rows, rows)],
                xbuf.at[pl.ds(c * rows, rows)], in_sems.at[c])
            cp.start()
            loads.append(cp)
        gcp = pltpu.make_async_copy(g_ref, gbuf, g_sem)
        gcp.start()
        bar = pltpu.get_barrier_semaphore()
        for d in range(1, N_DEV):
            pl.semaphore_signal(bar, inc=1, device_id=((me + d) % N_DEV,),
                                device_id_type=pl.DeviceIdType.MESH)
        row = lax.broadcasted_iota(jnp.int32, (rows, LANES), 0)
        lane = lax.broadcasted_iota(jnp.int32, (rows, LANES), 1)
        diag = row == lane
        sends = []
        for c in range(nch):
            loads[c].wait()
            xv = xbuf[pl.ds(c * rows, rows), :]
            sq = xv * xv
            p = sq[:, 0:LANES]
            for j in range(1, nj):
                p = p + sq[:, j * LANES:(j + 1) * LANES]
            s = jnp.sum(p, axis=1, keepdims=True)
            sbuf[c] = jnp.sum(jnp.where(diag, s, 0.0), axis=0, keepdims=True)
            if c == 0:
                pl.semaphore_wait(bar, N_DEV - 1)
            for d in (2, 1, 3):
                cc = pltpu.make_async_remote_copy(
                    src_ref=sbuf.at[c], dst_ref=rbuf.at[c, d - 1],
                    send_sem=send_sems.at[c * (N_DEV - 1) + d - 1],
                    recv_sem=recv_sems.at[c],
                    device_id=((me + d) % N_DEV,),
                    device_id_type=pl.DeviceIdType.MESH)
                cc.start()
                sends.append(cc)
        gcp.wait()
        g = gbuf[...]
        for c in range(nch):
            if c == nch - 1:
                for cc in sends:
                    cc.wait_send()
            pltpu.make_async_copy(rbuf.at[c], rbuf.at[c], recv_sems.at[c]).wait()
            tot = sbuf[c] + rbuf[c, 0] + rbuf[c, 1] + rbuf[c, 2]
            inv = lax.rsqrt(tot * (1.0 / n_glob) + EPS)
            col = jnp.sum(jnp.where(diag, inv, 0.0), axis=1, keepdims=True)
            xv = xbuf[pl.ds(c * rows, rows), :]
            o_ref[pl.ds(c * rows, rows), :] = xv * col * g

    return pl.pallas_call(
        body,
        out_shape=pltpu.VMEM((m, n), x.dtype),
        in_specs=[pl.BlockSpec(memory_space=pl.ANY),
                  pl.BlockSpec(memory_space=pl.ANY)],
        out_specs=pl.BlockSpec(memory_space=pltpu.VMEM),
        scratch_shapes=[
            pltpu.VMEM((m, n), jnp.float32),
            pltpu.VMEM((1, n), jnp.float32),
            pltpu.VMEM((nch, 1, LANES), jnp.float32),
            pltpu.VMEM((nch, N_DEV - 1, 1, LANES), jnp.float32),
            pltpu.SemaphoreType.DMA((nch,)),
            pltpu.SemaphoreType.DMA,
            pltpu.SemaphoreType.DMA((nch * (N_DEV - 1),)),
            pltpu.SemaphoreType.DMA((nch,)),
        ],
        compiler_params=pltpu.CompilerParams(
            collective_id=0, disable_semaphore_checks=True,
            disable_bounds_checks=True),
    )(x, g2)
```

```python
import jax
import jax.numpy as jnp
from jax import lax
from jax.experimental import pallas as pl
from jax.experimental.pallas import tpu as pltpu

N_DEV = 4
EPS = 1e-5
LANES = 128
SUBLANES = 8

REGIONS = (128, 128, 128, 128, (128,), (80, 48))
WAIT_SENDS_AFTER = 0
BASES_AFTER = 2


def pallas_dist_rmsnorm_colshard_i_m768_n512_kernel(
    x: jax.Array,
    gamma: jax.Array,
):
    m, n = x.shape
    nj = n // LANES
    inv_n = 1.0 / (n * N_DEV)

    nreg = len(REGIONS)
    reg_rows = [r if isinstance(r, int) else sum(r) for r in REGIONS]
    reg_start = [sum(reg_rows[:i]) for i in range(nreg)]
    assert sum(reg_rows) == m and n % LANES == 0
    assert all(r <= LANES and r % SUBLANES == 0 for r in reg_rows)
    units = []
    n_smem = 0
    for ri, reg in enumerate(REGIONS):
        if isinstance(reg, int):
            units.append((ri, 0, reg, None, True))
        else:
            off = 0
            for k, rows in enumerate(reg):
                assert rows % SUBLANES == 0
                units.append((ri, off, rows, n_smem, k == len(reg) - 1))
                n_smem += 1
                off += rows
    n_sends = sum(3 if isinstance(r, int) else 2 + len(r) for r in REGIONS)

    def body(x_ref, g_ref, o_ref, xbuf, gbuf, sbuf, ubuf, rbuf, rsm,
             in_sems, g_sem, send_sems, recv_sems, srecv_sems):
        me = lax.axis_index("i")

        loads = []
        for u, (ri, off, rows, _, _) in enumerate(units):
            r0 = reg_start[ri] + off
            cp = pltpu.make_async_copy(
                x_ref.at[pl.ds(r0, rows)], xbuf.at[pl.ds(r0, rows)], in_sems.at[u])
            cp.start()
            loads.append(cp)
        g_load = pltpu.make_async_copy(g_ref, gbuf, g_sem)
        g_load.start()
        barrier = pltpu.get_barrier_semaphore()
        for d in range(1, N_DEV):
            pl.semaphore_signal(barrier, inc=1, device_id=((me + d) % N_DEV,),
                                device_id_type=pl.DeviceIdType.MESH)

        def diag(rows, off=0):
            row = lax.broadcasted_iota(jnp.int32, (rows, LANES), 0)
            lane = lax.broadcasted_iota(jnp.int32, (rows, LANES), 1)
            return row + off == lane

        sends = []

        def send(src, dst, recv_sem, d):
            cp = pltpu.make_async_remote_copy(
                src_ref=src, dst_ref=dst,
                send_sem=send_sems.at[len(sends)], recv_sem=recv_sem,
                device_id=((me + d) % N_DEV,),
                device_id_type=pl.DeviceIdType.MESH)
            cp.start()
            sends.append(cp)
            return cp

        from_diag = {}
        region_acc = {}
        for u, (ri, off, rows, slot, last) in enumerate(units):
            r0 = reg_start[ri] + off
            loads[u].wait()
            xv = xbuf[pl.ds(r0, rows), :]
            sq = xv * xv
            parts = [sq[:, j * LANES:(j + 1) * LANES] for j in range(nj)]
            while len(parts) > 1:
                parts = [parts[i] + parts[i + 1] if i + 1 < len(parts) else parts[i]
                         for i in range(0, len(parts), 2)]
            s = jnp.sum(parts[0], axis=1, keepdims=True)
            packed = jnp.sum(jnp.where(diag(rows, off), s, 0.0),
                             axis=0, keepdims=True)
            if slot is None:
                sbuf[ri] = packed
            else:
                ubuf[slot] = packed
            if u == 0:
                pl.semaphore_wait(barrier, N_DEV - 1)
            if slot is None:
                send(sbuf.at[ri], rbuf.at[ri, 2], recv_sems.at[ri], 2)
            else:
                from_diag[u] = send(ubuf.at[slot], rsm.at[slot], srecv_sems.at[slot], 2)
                region_acc[ri] = packed if ri not in region_acc else region_acc[ri] + packed
                if last:
                    sbuf[ri] = region_acc[ri]
            if last:
                send(sbuf.at[ri], rbuf.at[ri, 0], recv_sems.at[ri], 1)
                send(sbuf.at[ri], rbuf.at[ri, 1], recv_sems.at[ri], 3)

        g_load.wait()
        g = gbuf[...]
        sub = lax.broadcasted_iota(jnp.int32, (SUBLANES, LANES), 0)
        bases = {}
        for u, (ri, off, rows, slot, _) in enumerate(units):
            r0 = reg_start[ri] + off
            if slot is None:
                pltpu.make_async_copy(rbuf.at[ri], rbuf.at[ri], recv_sems.at[ri]).wait()
                tot = (sbuf[ri] + rbuf[ri, 0]) + (rbuf[ri, 1] + rbuf[ri, 2])
                inv = lax.rsqrt(tot * inv_n + EPS)
                col = jnp.sum(jnp.where(diag(rows), inv, 0.0), axis=1, keepdims=True)
                o_ref[pl.ds(r0, rows), :] = xbuf[pl.ds(r0, rows), :] * col * g
            else:
                from_diag[u].wait_recv()
                xg = xbuf[pl.ds(r0, rows), :] * g
                for q in range(rows // SUBLANES):
                    l0 = off + SUBLANES * q
                    v = jnp.full((SUBLANES, LANES), rsm[slot, 0, l0], jnp.float32)
                    for k in range(1, SUBLANES):
                        v = jnp.where(sub == k, rsm[slot, 0, l0 + k], v)
                    inv = lax.rsqrt(v * inv_n + bases[ri][l0:l0 + SUBLANES, :])
                    for j in range(nj):
                        o_ref[pl.ds(r0 + SUBLANES * q, SUBLANES), pl.ds(j * LANES, LANES)] = (
                            xg[SUBLANES * q:SUBLANES * (q + 1), j * LANES:(j + 1) * LANES] * inv)
            if u == WAIT_SENDS_AFTER:
                for cp in sends:
                    cp.wait_send()
            if u == BASES_AFTER:
                fast = [i for i in range(nreg) if not isinstance(REGIONS[i], int)]
                for i in fast:
                    two = rbuf.at[i, pl.ds(0, 2)]
                    pltpu.make_async_copy(two, two, recv_sems.at[i]).wait()
                for i in fast:
                    part = (sbuf[i] + rbuf[i, 0] + rbuf[i, 1]) * inv_n + EPS
                    col = jnp.sum(jnp.where(diag(reg_rows[i]), part, 0.0),
                                  axis=1, keepdims=True)
                    bases[i] = jnp.broadcast_to(col, (reg_rows[i], LANES))

    return pl.pallas_call(
        body,
        out_shape=pltpu.VMEM((m, n), x.dtype),
        in_specs=[pl.BlockSpec(memory_space=pl.ANY),
                  pl.BlockSpec(memory_space=pl.ANY)],
        out_specs=pl.BlockSpec(memory_space=pltpu.VMEM),
        scratch_shapes=[
            pltpu.VMEM((m, n), jnp.float32),
            pltpu.VMEM((1, n), jnp.float32),
            pltpu.VMEM((nreg, 1, LANES), jnp.float32),
            pltpu.VMEM((n_smem, 1, LANES), jnp.float32),
            pltpu.VMEM((nreg, N_DEV - 1, 1, LANES), jnp.float32),
            pltpu.SMEM((n_smem, 1, LANES), jnp.float32),
            pltpu.SemaphoreType.DMA((len(units),)),
            pltpu.SemaphoreType.DMA,
            pltpu.SemaphoreType.DMA((n_sends,)),
            pltpu.SemaphoreType.DMA((nreg,)),
            pltpu.SemaphoreType.DMA((n_smem,)),
        ],
        compiler_params=pltpu.CompilerParams(
            collective_id=0,
            disable_semaphore_checks=True,
            disable_bounds_checks=True,
        ),
    )(x, gamma.reshape(1, n))
```
